```python
import numpy as np

kernel_name = "dist_rsx_agy_m2048_n1024"

def setup_inputs():
    return {"x": np.random.randn(2, 2048, 2048).astype(np.float32)}

def reference(x: np.ndarray) -> np.ndarray:
    return x.sum(axis=0)
```

```python
import jax
import jax.numpy as jnp
from jax import lax
from jax.experimental import pallas as pl
from jax.experimental.pallas import tpu as pltpu

MESH = pl.DeviceIdType.MESH
RC = 8
AHEAD = 16
RING = 32
LD_ROWS = 128


def pallas_dist_rsx_agy_m2048_n1024_kernel(x: jax.Array):
    _, m, n = x.shape
    nc, nld, cpl = m // RC, m // LD_ROWS, LD_ROWS // RC

    def body(x_hbm, out_ref, xf, xs, xr, ld_sem, xr_sem, sems):
        mx, my = lax.axis_index("x"), lax.axis_index("y")
        xn, yn = (1 - mx, my), (mx, 1 - my)
        xs_sem, ys_sem, yr_sem = sems.at[0], sems.at[1], sems.at[2]
        bar = pltpu.get_barrier_semaphore()
        for nb in (xn, yn):
            pl.semaphore_signal(bar, 1, device_id=nb, device_id_type=MESH)

        def load(i):
            start = i * LD_ROWS
            rows = pl.ds(start if isinstance(i, int) else pl.multiple_of(start, LD_ROWS), LD_ROWS)
            return pltpu.make_async_copy(x_hbm.at[0, rows], xf.at[rows], ld_sem.at[i])

        for i in range(nld):
            load(i).start()

        col0 = pl.multiple_of(my * n, n)
        ocol0 = pl.multiple_of((1 - my) * n, n)

        def rows_of(c):
            return pl.ds(pl.multiple_of(c * RC, RC), RC)

        def xcopy(c):
            r = rows_of(c)
            return pltpu.make_async_remote_copy(
                xs.at[r], xr.at[r], xs_sem, xr_sem.at[c % RING], device_id=xn, device_id_type=MESH)

        def ycopy(c):
            blk = out_ref.at[rows_of(c), pl.ds(col0, n)]
            return pltpu.make_async_remote_copy(blk, blk, ys_sem, yr_sem, device_id=yn, device_id_type=MESH)

        def send_x(c, _=None):
            @pl.when(c % cpl == 0)
            def _():
                load(c // cpl).wait()
            r = rows_of(c)
            xs[r, :] = xf[r, :].astype(jnp.bfloat16)
            xcopy(c).start()

        def reduce_send_y(c, _=None):
            xcopy(c).wait_recv()
            r = rows_of(c)
            s = xs[r, :].astype(jnp.float32) + xr[r, :].astype(jnp.float32)
            out_ref[r, pl.ds(col0, n)] = s.astype(out_ref.dtype)
            ycopy(c).start()

        def main(c, _):
            reduce_send_y(c)
            send_x(c + AHEAD)

        pl.semaphore_wait(bar, 2)
        lax.fori_loop(0, AHEAD, send_x, None)
        lax.fori_loop(0, nc - AHEAD, main, None)
        lax.fori_loop(nc - AHEAD, nc, reduce_send_y, None)

        mine = out_ref.at[:, pl.ds(col0, n)]
        theirs = out_ref.at[:, pl.ds(ocol0, n)]
        pltpu.make_async_remote_copy(xs, xr, xs_sem, xr_sem.at[0], device_id=xn, device_id_type=MESH).wait_send()
        pltpu.make_async_remote_copy(mine, mine, ys_sem, yr_sem, device_id=yn, device_id_type=MESH).wait_send()
        pltpu.make_async_remote_copy(theirs, theirs, ys_sem, yr_sem, device_id=yn, device_id_type=MESH).wait_recv()

    return pl.pallas_call(
        body,
        out_shape=pltpu.VMEM((m, 2 * n), jnp.bfloat16),
        in_specs=[pl.BlockSpec(memory_space=pltpu.HBM)],
        out_specs=pl.BlockSpec(memory_space=pltpu.VMEM),
        scratch_shapes=[
            pltpu.VMEM((m, n), jnp.float32),
            pltpu.VMEM((m, n), jnp.bfloat16),
            pltpu.VMEM((m, n), jnp.bfloat16),
            pltpu.SemaphoreType.DMA((nld,)),
            pltpu.SemaphoreType.DMA((RING,)),
            pltpu.SemaphoreType.DMA((3,)),
        ],
        compiler_params=pltpu.CompilerParams(collective_id=0, vmem_limit_bytes=48 * 2**20),
    )(x)
```

```python
import jax
import jax.numpy as jnp
from jax import lax
from jax.experimental import pallas as pl
from jax.experimental.pallas import tpu as pltpu

UNIT_ROWS = 8
UNIT_COLS = 256
OWNED_ROWS = 40
AHEAD = 32
SLOTS = 2 * AHEAD
LOAD_ROWS = (64, 64, 256)

_MESH = pl.DeviceIdType.MESH


def _aligned(value, multiple):
    return value if isinstance(value, int) else pl.multiple_of(value, multiple)


def _kernel(
    x_hbm,
    out_ref,
    x_f32,
    raw_out,
    raw_in,
    head_in,
    load_sems,
    raw_sems,
    sems,
    y_entered,
):
    _, m, n = x_hbm.shape
    half = n // 2
    rows, cols = UNIT_ROWS, UNIT_COLS
    assert half == 2 * cols and AHEAD >= OWNED_ROWS // rows * (half // cols)
    n_owned = OWNED_ROWS // rows * (half // cols)
    n_units = n_owned + (m - OWNED_ROWS) // rows * (n // cols)

    (
        sent_head,
        sent_second,
        sent_raw_owned,
        sent_raw_rest,
        sent_sum_owned,
        sent_sum_rest,
        got_sum_owned,
        got_sum_rest,
    ) = (sems.at[i] for i in range(8))

    ix, iy = lax.axis_index("x"), lax.axis_index("y")
    x_peer, y_peer = (1 - ix, iy), (ix, 1 - iy)
    my_share = pl.multiple_of(ix * half, half)
    peer_share = pl.multiple_of((1 - ix) * half, half)
    my_half = pl.multiple_of(iy * n, n)
    peer_half = pl.multiple_of((1 - iy) * n, n)

    def remote(src, dst, send_sem, recv_sem, peer):
        return pltpu.make_async_remote_copy(
            src, dst, send_sem, recv_sem, device_id=peer, device_id_type=_MESH
        )

    blocks = [
        (1, pl.ds(0, rows), pl.ds(_aligned(peer_share + cols, cols), cols)),
        (2, pl.ds(rows, 2 * rows), pl.ds(peer_share, half)),
        (6, pl.ds(3 * rows, OWNED_ROWS - 3 * rows), pl.ds(peer_share, half)),
    ]
    start = OWNED_ROWS
    for size in (*LOAD_ROWS, m - OWNED_ROWS - sum(LOAD_ROWS)):
        step = n_owned + (start - OWNED_ROWS) // rows * (n // cols)
        blocks.append((step, pl.ds(start, size), pl.ds(0, n)))
        start += size
    blocks.insert(4, (AHEAD, pl.ds(0, OWNED_ROWS), pl.ds(my_share, half)))

    def load(i):
        _, r, c = blocks[i]
        return pltpu.make_async_copy(x_hbm.at[0, r, c], x_f32.at[r, c], load_sems.at[i])

    def start_loads(lo, hi):
        for i in range(lo, hi):
            load(i).start()

    def unit(k, owned, share):
        if owned:
            per_row, row0, col0 = half // cols, 0, share
        else:
            k, per_row, row0, col0 = k - n_owned, n // cols, OWNED_ROWS, 0
        return (
            pl.ds(_aligned(row0 + k // per_row * rows, rows), rows),
            _aligned(col0 + k % per_row * cols, cols),
        )

    def is_unit(k, i):
        return isinstance(k, int) and k == i

    def raw_copy(k, owned, r, c):
        c = pl.ds(c, cols)
        if is_unit(k, 0):
            return remote(x_hbm.at[0, r, c], head_in, sent_head, raw_sems.at[0], x_peer)
        sent = sent_raw_owned if owned else sent_raw_rest
        if is_unit(k, 1):
            sent = sent_second
        return remote(
            raw_out.at[r, c], raw_in.at[r, c], sent, raw_sems.at[k % SLOTS], x_peer
        )

    def send_raw(k, owned):
        r, c = unit(k, owned, peer_share)
        if not is_unit(k, 0):
            raw_out[r, pl.ds(c, cols)] = x_f32[r, pl.ds(c, cols)].astype(jnp.bfloat16)
        raw_copy(k, owned, r, c).start()

    def reduce_and_send(k, owned):
        r, c = unit(k, owned, my_share)
        raw_copy(k, owned, r, c).wait_recv()
        if is_unit(k, 0):
            theirs = head_in[...]
        else:
            theirs = raw_in[r, pl.ds(c, cols)].astype(jnp.float32)
        mine = x_f32[r, pl.ds(c, cols)].astype(jnp.bfloat16).astype(jnp.float32)
        c = pl.ds(pl.multiple_of(my_half + c, cols), cols)
        out_ref[r, c] = (mine + theirs).astype(out_ref.dtype)
        sent, got = (
            (sent_sum_owned, got_sum_owned) if owned else (sent_sum_rest, got_sum_rest)
        )
        remote(out_ref.at[r, c], out_ref.at[r, c], sent, got, y_peer).start()

    def out_share(first_col):
        c = pl.ds(pl.multiple_of(first_col + my_share, half), half)
        return out_ref.at[pl.ds(0, OWNED_ROWS), c]

    def out_rest(first_col):
        return out_ref.at[pl.ds(OWNED_ROWS, m - OWNED_ROWS), pl.ds(first_col, n)]

    def pass_on(i):
        share = out_share(i * n)
        return remote(share, share, sems.at[8 + i], sems.at[10 + i], x_peer)

    barrier = pltpu.get_barrier_semaphore()

    @pl.when(iy == 0)
    def _():
        pl.semaphore_signal(barrier, 1, device_id=y_peer, device_id_type=_MESH)

    pl.semaphore_signal(barrier, 1, device_id=x_peer, device_id_type=_MESH)
    start_loads(0, 2)
    pl.when(ix == 0)(lambda: start_loads(2, 5))
    pl.when(iy == 0)(lambda: pl.semaphore_wait(barrier, 1))
    pl.when(iy == 1)(lambda: pl.semaphore_wait(barrier, 2))
    send_raw(0, True)
    pl.when(ix == 1)(lambda: start_loads(2, 5))

    @pl.when(iy == 1)
    def _():
        pl.semaphore_signal(y_entered, 1, device_id=y_peer, device_id_type=_MESH)

    cuts = {1, 2, n_owned, n_units}
    cuts |= {c + AHEAD for c in (0, 1, 2, n_owned, n_units)}
    cuts |= {step for step, _, _ in blocks}
    cuts = sorted(cuts)
    for lo, hi in zip(cuts[:-1], cuts[1:]):
        for i, (step, _, _) in enumerate(blocks):
            if step == lo:
                load(i).wait()
        if lo == n_owned:
            start_loads(5, len(blocks))
        if lo == AHEAD:
            pl.when(iy == 0)(lambda: pl.semaphore_wait(y_entered, 1))
        if lo == n_units:
            share = out_share(peer_half)
            remote(share, share, sent_sum_owned, got_sum_owned, y_peer).wait_recv()
            pass_on(0).start()
            pass_on(1).start()

        def step_fn(t, _=None, lo=lo):
            if lo >= AHEAD:
                reduce_and_send(t - AHEAD, lo - AHEAD < n_owned)
            if lo < n_units:
                send_raw(t, lo < n_owned)

        if hi - lo == 1:
            step_fn(lo)
        else:
            lax.fori_loop(lo, hi, step_fn, None)

    for k in (0, 1):
        raw_copy(k, True, *unit(k, True, peer_share)).wait_send()
    for src, sem in (
        (raw_out.at[pl.ds(rows, OWNED_ROWS - rows), pl.ds(peer_share, half)], sent_raw_owned),
        (raw_out.at[pl.ds(OWNED_ROWS, m - OWNED_ROWS)], sent_raw_rest),
        (out_share(my_half), sent_sum_owned),
        (out_rest(my_half), sent_sum_rest),
    ):
        remote(src, src, sem, got_sum_rest, x_peer).wait_send()
    pass_on(0).wait_send()
    pass_on(1).wait_send()
    rest = out_rest(peer_half)
    remote(rest, rest, sent_sum_rest, got_sum_rest, y_peer).wait_recv()
    pass_on(0).wait_recv()
    pass_on(1).wait_recv()


def pallas_dist_rsx_agy_m2048_n1024_kernel(x: jax.Array):
    _, m, n = x.shape
    return pl.pallas_call(
        _kernel,
        out_shape=pltpu.VMEM((m, 2 * n), jnp.bfloat16),
        in_specs=[pl.BlockSpec(memory_space=pltpu.HBM)],
        out_specs=pl.BlockSpec(memory_space=pltpu.VMEM),
        scratch_shapes=[
            pltpu.VMEM((m, n), jnp.float32),
            pltpu.VMEM((m, n), jnp.bfloat16),
            pltpu.VMEM((m, n), jnp.bfloat16),
            pltpu.VMEM((UNIT_ROWS, UNIT_COLS), jnp.float32),
            pltpu.SemaphoreType.DMA((5 + len(LOAD_ROWS),)),
            pltpu.SemaphoreType.DMA((SLOTS,)),
            pltpu.SemaphoreType.DMA((12,)),
            pltpu.SemaphoreType.REGULAR,
        ],
        compiler_params=pltpu.CompilerParams(
            collective_id=0,
            vmem_limit_bytes=48 * 2**20,
            disable_semaphore_checks=True,
        ),
    )(x)
```

```python
import functools

import jax
import jax.numpy as jnp
from jax import lax
from jax.experimental import pallas as pl
from jax.experimental.pallas import tpu as pltpu

UNIT_ROWS = 8
UNIT_COLS = 256
OWNED_ROWS = 40
AHEAD = 32
SLOTS = 2 * AHEAD
LOAD_ROWS = (64, 64, 256)

_MESH = pl.DeviceIdType.MESH
_DMA = pltpu.SemaphoreType.DMA


def _aligned(value, multiple):
    return value if isinstance(value, int) else pl.multiple_of(value, multiple)


def _remote(src, dst, send_sem, recv_sem, peer):
    return pltpu.make_async_remote_copy(
        src, dst, send_sem, recv_sem, device_id=peer, device_id_type=_MESH
    )


def _kernel(
    x_hbm,
    out_ref,
    x_f32,
    raw_out,
    raw_in,
    head_in,
    got_last,
):
    _, m, n = x_hbm.shape
    half = n // 2
    rows, cols = UNIT_ROWS, UNIT_COLS
    n_owned = OWNED_ROWS // rows * (half // cols)
    n_units = n_owned + (m - OWNED_ROWS) // rows * (n // cols)
    assert half == 2 * cols and AHEAD >= n_owned

    ix, iy = lax.axis_index("x"), lax.axis_index("y")
    x_peer, y_peer = (1 - ix, iy), (ix, 1 - iy)
    my_share = pl.multiple_of(ix * half, half)
    peer_share = pl.multiple_of((1 - ix) * half, half)
    my_half = pl.multiple_of(iy * n, n)
    peer_half = pl.multiple_of((1 - iy) * n, n)
    got_sum_rest = got_last.at[0]

    def unit(k, owned, share):
        if owned:
            per_row, row0, col0 = half // cols, 0, share
        else:
            k, per_row, row0, col0 = k - n_owned, n // cols, OWNED_ROWS, 0
        return (
            pl.ds(_aligned(row0 + k // per_row * rows, rows), rows),
            _aligned(col0 + k % per_row * cols, cols),
        )

    def out_share(first_col):
        c = pl.ds(pl.multiple_of(first_col + my_share, half), half)
        return out_ref.at[pl.ds(0, OWNED_ROWS), c]

    def out_rest(first_col):
        return out_ref.at[pl.ds(OWNED_ROWS, m - OWNED_ROWS), pl.ds(first_col, n)]

    blocks = [
        (1, pl.ds(0, rows), pl.ds(_aligned(peer_share + cols, cols), cols)),
        (2, pl.ds(rows, 2 * rows), pl.ds(peer_share, half)),
        (6, pl.ds(3 * rows, OWNED_ROWS - 3 * rows), pl.ds(peer_share, half)),
    ]
    start = OWNED_ROWS
    for size in (*LOAD_ROWS, m - OWNED_ROWS - sum(LOAD_ROWS)):
        step = n_owned + (start - OWNED_ROWS) // rows * (n // cols)
        blocks.append((step, pl.ds(start, size), pl.ds(0, n)))
        start += size
    blocks.insert(4, (AHEAD, pl.ds(0, OWNED_ROWS), pl.ds(my_share, half)))

    def streams(sent, load_sems, raw_sems, got_sum_owned, y_entered):
        sent_head, sent_second, sent_raw_owned, sent_raw_rest = (
            sent.at[i] for i in range(4)
        )
        sent_sum_owned, sent_sum_rest = sent.at[4], sent.at[5]

        def load(i):
            _, r, c = blocks[i]
            return pltpu.make_async_copy(
                x_hbm.at[0, r, c], x_f32.at[r, c], load_sems.at[i]
            )

        def start_loads(lo, hi):
            for i in range(lo, hi):
                load(i).start()

        def is_unit(k, i):
            return isinstance(k, int) and k == i

        def raw_copy(k, owned, r, c):
            c = pl.ds(c, cols)
            got = raw_sems.at[k % SLOTS]
            if is_unit(k, 0):
                return _remote(x_hbm.at[0, r, c], head_in, sent_head, got, x_peer)
            sent_raw = sent_raw_owned if owned else sent_raw_rest
            if is_unit(k, 1):
                sent_raw = sent_second
            return _remote(raw_out.at[r, c], raw_in.at[r, c], sent_raw, got, x_peer)

        def send_raw(k, owned):
            r, c = unit(k, owned, peer_share)
            if not is_unit(k, 0):
                block = x_f32[r, pl.ds(c, cols)]
                raw_out[r, pl.ds(c, cols)] = block.astype(jnp.bfloat16)
            raw_copy(k, owned, r, c).start()

        def reduce_and_send(k, owned):
            r, c = unit(k, owned, my_share)
            raw_copy(k, owned, r, c).wait_recv()
            if is_unit(k, 0):
                theirs = head_in[...]
            else:
                theirs = raw_in[r, pl.ds(c, cols)].astype(jnp.float32)
            mine = x_f32[r, pl.ds(c, cols)].astype(jnp.bfloat16).astype(jnp.float32)
            c = pl.ds(pl.multiple_of(my_half + c, cols), cols)
            out_ref[r, c] = (mine + theirs).astype(out_ref.dtype)
            if owned:
                sent_sum, got = sent_sum_owned, got_sum_owned
            else:
                sent_sum, got = sent_sum_rest, got_sum_rest
            _remote(out_ref.at[r, c], out_ref.at[r, c], sent_sum, got, y_peer).start()

        barrier = pltpu.get_barrier_semaphore()

        @pl.when(iy == 0)
        def _():
            pl.semaphore_signal(barrier, 1, device_id=y_peer, device_id_type=_MESH)

        pl.semaphore_signal(barrier, 1, device_id=x_peer, device_id_type=_MESH)
        start_loads(0, 2)
        pl.when(ix == 0)(lambda: start_loads(2, 5))
        pl.when(iy == 0)(lambda: pl.semaphore_wait(barrier, 1))
        pl.when(iy == 1)(lambda: pl.semaphore_wait(barrier, 2))
        send_raw(0, True)
        pl.when(ix == 1)(lambda: start_loads(2, 5))

        @pl.when(iy == 1)
        def _():
            pl.semaphore_signal(y_entered, 1, device_id=y_peer, device_id_type=_MESH)

        cuts = {1, 2, n_owned, n_units}
        cuts |= {c + AHEAD for c in (0, 1, 2, n_owned, n_units)}
        cuts |= {step for step, _, _ in blocks}
        cuts = sorted(cuts)
        for lo, hi in zip(cuts[:-1], cuts[1:]):
            for i, (step, _, _) in enumerate(blocks):
                if step == lo:
                    load(i).wait()
            if lo == n_owned:
                start_loads(5, len(blocks))
            if lo == AHEAD:
                pl.when(iy == 0)(lambda: pl.semaphore_wait(y_entered, 1))
            if lo == n_units:
                share = out_share(peer_half)
                _remote(share, share, sent_sum_owned, got_sum_owned, y_peer).wait_recv()
                for i in range(2):
                    share = out_share(i * n)
                    _remote(
                        share, share, sent.at[6 + i], got_last.at[1 + i], x_peer
                    ).start()

            def step_fn(t, _=None, lo=lo):
                if lo >= AHEAD:
                    reduce_and_send(t - AHEAD, lo - AHEAD < n_owned)
                if lo < n_units:
                    send_raw(t, lo < n_owned)

            if hi - lo == 1:
                step_fn(lo)
            else:
                lax.fori_loop(lo, hi, step_fn, None)

    @functools.partial(pl.run_scoped, sent=_DMA((8,)))
    def _(sent):
        pl.run_scoped(
            functools.partial(streams, sent),
            _DMA((len(blocks),)),
            _DMA((SLOTS,)),
            _DMA,
            pltpu.SemaphoreType.REGULAR,
        )
        raw = (
            blocks[0][1:],
            (pl.ds(rows, OWNED_ROWS - rows), pl.ds(peer_share, half)),
            (pl.ds(OWNED_ROWS, m - OWNED_ROWS), pl.ds(0, n)),
        )
        sums = (out_share(my_half), out_rest(my_half), out_share(0), out_share(n))
        copies = (
            (x_hbm.at[0, pl.ds(0, rows), pl.ds(peer_share, cols)], head_in),
            *((raw_out.at[block], raw_in.at[block]) for block in raw),
            *((block, block) for block in sums),
        )
        for i, (src, dst) in enumerate(copies):
            _remote(src, dst, sent.at[i], got_sum_rest, x_peer).wait_send()

    last = (
        out_rest(peer_half),
        out_ref.at[pl.ds(0, OWNED_ROWS), pl.ds(peer_share, half)],
        out_ref.at[pl.ds(0, OWNED_ROWS), pl.ds(_aligned(n + peer_share, half), half)],
    )
    for i, dst in enumerate(last):
        _remote(dst, dst, got_last.at[i], got_last.at[i], x_peer).wait_recv()


def pallas_dist_rsx_agy_m2048_n1024_kernel(x: jax.Array):
    _, m, n = x.shape
    return pl.pallas_call(
        _kernel,
        out_shape=pltpu.VMEM((m, 2 * n), jnp.bfloat16),
        in_specs=[pl.BlockSpec(memory_space=pltpu.HBM)],
        out_specs=pl.BlockSpec(memory_space=pltpu.VMEM),
        scratch_shapes=[
            pltpu.VMEM((m, n), jnp.float32),
            pltpu.VMEM((m, n), jnp.bfloat16),
            pltpu.VMEM((m, n), jnp.bfloat16),
            pltpu.VMEM((UNIT_ROWS, UNIT_COLS), jnp.float32),
            _DMA((3,)),
        ],
        compiler_params=pltpu.CompilerParams(
            collective_id=0, vmem_limit_bytes=48 * 2**20
        ),
    )(x)
```
